```python
import numpy as np

kernel_name = "dist_rope_attn_htp_bs_b2_sq512_d1024_hq8_dh128"

def setup_inputs():
    x = np.random.randn(8, 512, 1024).astype(np.float32)
    Wq = np.random.randn(1024, 4096).astype(np.float32) * 0.02
    Wk = np.random.randn(1024, 4096).astype(np.float32) * 0.02
    Wv = np.random.randn(1024, 4096).astype(np.float32) * 0.02
    Wo = np.random.randn(4096, 1024).astype(np.float32) * 0.02
    return {"x": x, "Wq": Wq, "Wk": Wk, "Wv": Wv, "Wo": Wo}

def reference(x, Wq, Wk, Wv, Wo):
    B, Sq, Hq, Dh = 8, 512, 32, 128
    inv = 1.0 / (10000.0 ** (np.arange(0, Dh, 2) / Dh))
    pos = np.arange(Sq)[:, None] * inv[None, :]
    cos = np.repeat(np.cos(pos), 2, axis=-1).astype(np.float32)
    sin = np.repeat(np.sin(pos), 2, axis=-1).astype(np.float32)
    def rot(t):
        t2 = t.reshape(B, Sq, Hq, Dh // 2, 2)
        t_r = np.stack([-t2[..., 1], t2[..., 0]], axis=-1).reshape(B, Sq, Hq, Dh)
        return t * cos[None, :, None, :] + t_r * sin[None, :, None, :]
    Q = rot((x @ Wq).reshape(B, Sq, Hq, Dh))
    K = rot((x @ Wk).reshape(B, Sq, Hq, Dh))
    V = (x @ Wv).reshape(B, Sq, Hq, Dh)
    s = np.einsum('bihd,bjhd->bhij', Q, K).astype(np.float32) * 0.08838834764831843
    s_max = s.max(axis=-1, keepdims=True)
    w = np.exp(s - s_max)
    w = w / w.sum(axis=-1, keepdims=True)
    ctx = np.einsum('bhij,bjhd->bihd', w, V).reshape(B, Sq, Hq * Dh)
    return ctx @ Wo
```

```python
import numpy as np
import jax
import jax.numpy as jnp
from jax import lax
from jax.experimental import pallas as pl
from jax.experimental.pallas import tpu as pltpu

N_DEV = 4
SQ = 512
D = 1024
DH = 128
HL = 8
SCALE = 0.08838834764831843
LOG2E = 1.4426950408889634
BF = jnp.bfloat16
F32 = jnp.float32
MESH = pl.DeviceIdType.MESH


def _rope_tables():
    inv = 1.0 / (10000.0 ** (np.arange(0, DH, 2) / DH))
    pos = np.arange(SQ)[:, None] * inv[None, :]
    cos = np.repeat(np.cos(pos), 2, axis=-1)
    sin = np.repeat(np.sin(pos), 2, axis=-1)
    sign = np.where(np.arange(DH) % 2 == 0, -1.0, 1.0)[None, :]
    sin = sin * sign
    c = SCALE * LOG2E
    return np.stack([cos * c, sin * c, cos, sin]).astype(np.float32)


_TABLES = _rope_tables()


def _body(x_hbm, wq_hbm, wk_hbm, wv_hbm, wo_hbm, tab_hbm, out_hbm,
          xf, xg, wst, wqkv, wo, tab, ctx, sbuf, rbuf, acc0, ost,
          ld_sem, w_sem, xs_sem, xr_sem, ps_sem, pr_sem, o_sem):
    me = lax.axis_index("i")
    left = (me + N_DEV - 1) % N_DEV
    right = (me + 1) % N_DEV

    x_ld = [pltpu.make_async_copy(x_hbm.at[b], xf.at[b], ld_sem.at[b]) for b in range(2)]
    tab_ld = pltpu.make_async_copy(tab_hbm, tab, ld_sem.at[2])
    w_hbms = (wq_hbm, wk_hbm, wv_hbm)

    def w_ld(j, t):
        cols = pl.ds(j * 256, 256)
        return pltpu.make_async_copy(w_hbms[t].at[:, cols], wst.at[t, :, cols], w_sem.at[j * 3 + t])

    wo_ld = pltpu.make_async_copy(wo_hbm, wst.at[3], w_sem.at[12])

    x_ld[0].start()
    for t in range(3):
        w_ld(0, t).start()
    x_ld[1].start()
    tab_ld.start()
    for j in range(1, 4):
        for t in range(3):
            w_ld(j, t).start()
    wo_ld.start()

    barrier = pltpu.get_barrier_semaphore()
    for nbr in (left, right):
        pl.semaphore_signal(barrier, inc=1, device_id=(nbr,), device_id_type=MESH)

    def x_copy(src_slot, dst_slot, dev, k):
        return pltpu.make_async_remote_copy(
            src_ref=xg.at[src_slot], dst_ref=xg.at[dst_slot],
            send_sem=xs_sem.at[k], recv_sem=xr_sem.at[dst_slot],
            device_id=(dev,), device_id_type=MESH)

    x_sends = [
        x_copy(7, 1, right, 0), x_copy(0, 2, left, 1),
        x_copy(1, 4, right, 2), x_copy(2, 3, left, 3),
        x_copy(0, 5, right, 4), x_copy(7, 6, left, 5),
    ]

    def p_copy(k, dev):
        return pltpu.make_async_remote_copy(
            src_ref=sbuf.at[k], dst_ref=rbuf.at[k],
            send_sem=ps_sem.at[k], recv_sem=pr_sem.at[k],
            device_id=(dev,), device_id_type=MESH)

    rbuf[6] = jnp.zeros((SQ, D), BF)
    x_ld[0].wait()
    xg[0] = xf[0].astype(BF)
    pl.semaphore_wait(barrier, 2)
    x_sends[1].start()
    x_ld[1].wait()
    xg[7] = xf[1].astype(BF)
    x_sends[0].start()
    tab_ld.wait()

    even = (lax.broadcasted_iota(jnp.int32, (SQ, DH), 1) % 2) == 0

    def rope(t, c, s):
        sw = jnp.where(even, pltpu.roll(t, DH - 1, 1), pltpu.roll(t, 1, 1))
        return (t * c + sw * s).astype(BF)

    def head(xb, h):
        qkv = jnp.dot(xb, wqkv[h], preferred_element_type=F32)
        q = rope(qkv[:, 0:DH], tab[0], tab[1])
        k = rope(qkv[:, DH:2 * DH], tab[2], tab[3])
        v = qkv[:, 2 * DH:].astype(BF)
        s = lax.dot_general(q, k, (((1,), (1,)), ((), ())), preferred_element_type=F32)
        m = jnp.max(s, axis=-1, keepdims=True)
        p = jnp.exp2(s - m)
        l = jnp.sum(p, axis=-1, keepdims=True)
        o = jnp.dot(p.astype(BF), v, preferred_element_type=F32)
        ctx[:, h * DH:(h + 1) * DH] = (o * (1.0 / l)).astype(BF)

    def attn(slot, first=False):
        xb = xg[slot]
        for h in range(HL):
            if first and h % 2 == 0:
                j = h // 2
                for t in range(3):
                    w_ld(j, t).wait()
                    for hh in range(2):
                        c0 = j * 256 + hh * DH
                        wqkv[h + hh, :, t * DH:(t + 1) * DH] = wst[t, :, c0:c0 + DH].astype(BF)
            head(xb, h)

    NC = 2
    CW = D // NC

    def proj(c):
        return jnp.dot(ctx[...], wo[:, c * CW:(c + 1) * CW], preferred_element_type=F32)

    attn(0, first=True)
    wo_ld.wait()
    wo[...] = wst[3].astype(BF)
    for c in range(NC):
        acc0[:, c * CW:(c + 1) * CW] = proj(c)

    def step(s, carry):
        @pl.when(s == 1)
        def _():
            x_sends[0].wait_recv()
            x_sends[2].start()
            x_sends[1].wait_recv()
            x_sends[3].start()
            x_sends[4].start()
            x_sends[5].start()

        @pl.when(s >= 3)
        def _():
            x_copy(0, s, right, 0).wait_recv()

        @pl.when(s >= 5)
        def _():
            p_copy(s - 3, right).wait_recv()

        attn(s)
        add_slot = jnp.where(s >= 5, s - 3, 6)
        for c in range(NC):
            cols = slice(c * CW, (c + 1) * CW)
            sbuf[s - 1, :, cols] = (proj(c) + rbuf[add_slot, :, cols].astype(F32)).astype(BF)
        p_copy(s - 1, jnp.where(s % 2 == 1, left, right)).start()
        return carry

    lax.fori_loop(1, 7, step, 0)

    p_copy(1, right).wait_recv()
    p_copy(4, right).wait_recv()
    ost[0] = acc0[...] + rbuf[1].astype(F32) + rbuf[4].astype(F32)
    o_st0 = pltpu.make_async_copy(ost.at[0], out_hbm.at[0], o_sem.at[0])
    o_st0.start()
    attn(7)
    p_copy(0, right).wait_recv()
    p_copy(5, right).wait_recv()
    o_st = []
    for c in range(NC):
        cols = slice(c * CW, (c + 1) * CW)
        ost[1, :, cols] = proj(c) + rbuf[0, :, cols].astype(F32) + rbuf[5, :, cols].astype(F32)
        cp = pltpu.make_async_copy(ost.at[1, :, pl.ds(c * CW, CW)],
                                   out_hbm.at[1, :, pl.ds(c * CW, CW)], o_sem.at[1 + c])
        cp.start()
        o_st.append(cp)
    for cp in x_sends:
        cp.wait_send()
    for k in range(6):
        p_copy(k, right).wait_send()
    o_st0.wait()
    for cp in o_st:
        cp.wait()


def pallas_dist_rope_attn_htp_bs_b2_sq512_d1024_hq8_dh128_kernel(x, Wq, Wk, Wv, Wo):
    any_spec = pl.BlockSpec(memory_space=pl.ANY)
    return pl.pallas_call(
        _body,
        out_shape=jax.ShapeDtypeStruct((2, SQ, D), F32),
        in_specs=[any_spec] * 6,
        out_specs=any_spec,
        scratch_shapes=[
            pltpu.VMEM((2, SQ, D), F32),
            pltpu.VMEM((8, SQ, D), BF),
            pltpu.VMEM((4, D, D), F32),
            pltpu.VMEM((HL, D, 3 * DH), BF),
            pltpu.VMEM((D, D), BF),
            pltpu.VMEM((4, SQ, DH), F32),
            pltpu.VMEM((SQ, D), BF),
            pltpu.VMEM((6, SQ, D), BF),
            pltpu.VMEM((7, SQ, D), BF),
            pltpu.VMEM((SQ, D), F32),
            pltpu.VMEM((2, SQ, D), F32),
            pltpu.SemaphoreType.DMA((3,)),
            pltpu.SemaphoreType.DMA((13,)),
            pltpu.SemaphoreType.DMA((6,)),
            pltpu.SemaphoreType.DMA((8,)),
            pltpu.SemaphoreType.DMA((6,)),
            pltpu.SemaphoreType.DMA((6,)),
            pltpu.SemaphoreType.DMA((3,)),
        ],
        compiler_params=pltpu.CompilerParams(
            collective_id=0, vmem_limit_bytes=100 * 1024 * 1024),
    )(x, Wq, Wk, Wv, Wo, jnp.asarray(_TABLES))
```

```python
import numpy as np
import jax
import jax.numpy as jnp
from jax import lax
from jax.experimental import pallas as pl
from jax.experimental.pallas import tpu as pltpu

N_DEV = 4
SQ = 512
D = 1024
DH = 128
HL = 8
SCALE = 0.08838834764831843
LOG2E = 1.4426950408889634
BF = jnp.bfloat16
F32 = jnp.float32
MESH = pl.DeviceIdType.MESH


def _body(x_hbm, wq_hbm, wk_hbm, wv_hbm, wo_hbm, out_ref,
          xf, xg, wst, wqkv, wo, tab, ctx, sbuf, rbuf, acc0,
          ld_sem, w_sem, xs_sem, xr_sem, ps_sem, pr_sem):
    me = lax.axis_index("i")
    left = (me + N_DEV - 1) % N_DEV
    right = (me + 1) % N_DEV

    x_ld = [pltpu.make_async_copy(x_hbm.at[b], xf.at[b], ld_sem.at[b]) for b in range(2)]
    w_hbms = (wq_hbm, wk_hbm, wv_hbm)

    def w_ld(j, t):
        cols = pl.ds(j * 256, 256)
        return pltpu.make_async_copy(w_hbms[t].at[:, cols], wst.at[t, :, cols], w_sem.at[j * 3 + t])

    wo_ld = pltpu.make_async_copy(wo_hbm, wst.at[3], w_sem.at[12])

    x_ld[0].start()
    for t in range(3):
        w_ld(0, t).start()

    barrier = pltpu.get_barrier_semaphore()
    for nbr in (left, right):
        pl.semaphore_signal(barrier, inc=1, device_id=(nbr,), device_id_type=MESH)

    def x_copy(src_slot, dst_slot, dev, k):
        return pltpu.make_async_remote_copy(
            src_ref=xg.at[src_slot], dst_ref=xg.at[dst_slot],
            send_sem=xs_sem.at[k], recv_sem=xr_sem.at[dst_slot],
            device_id=(dev,), device_id_type=MESH)

    x_sends = [
        x_copy(7, 1, right, 0), x_copy(0, 2, left, 1),
        x_copy(1, 4, right, 2), x_copy(2, 3, left, 3),
        x_copy(0, 5, right, 4), x_copy(7, 6, left, 5),
    ]

    NC = 2
    CW = D // NC

    def p_copy(k, c, dev):
        cols = pl.ds(c * CW, CW)
        return pltpu.make_async_remote_copy(
            src_ref=sbuf.at[k, :, cols], dst_ref=rbuf.at[k, :, cols],
            send_sem=ps_sem.at[k * NC + c], recv_sem=pr_sem.at[k * NC + c],
            device_id=(dev,), device_id_type=MESH)

    def angles(n, mult):
        lane = lax.broadcasted_iota(jnp.int32, (n, DH), 1)
        row = lax.broadcasted_iota(jnp.int32, (n, DH), 0)
        inv = jnp.exp((lane // 2).astype(F32) * (-2.0 * np.log(10000.0) / DH))
        ang = (row * mult).astype(F32) * inv
        return jnp.cos(ang), jnp.sin(ang)

    ca, sa = (t[:, None, :] for t in angles(SQ // 8, 8))
    cb, sb = (t[None, :, :] for t in angles(8, 1))
    cos = (ca * cb - sa * sb).reshape(SQ, DH)
    sin = (sa * cb + ca * sb).reshape(SQ, DH)
    even = (lax.broadcasted_iota(jnp.int32, (SQ, DH), 1) % 2) == 0
    sin = jnp.where(even, -sin, sin)
    tab[0] = cos * (SCALE * LOG2E)
    tab[1] = sin * (SCALE * LOG2E)
    tab[2] = cos
    tab[3] = sin

    rbuf[6] = jnp.zeros((SQ, D), BF)
    x_ld[0].wait()
    x_ld[1].start()
    xg[0] = xf[0].astype(BF)
    pl.semaphore_wait(barrier, 2)
    x_sends[1].start()

    def rope(t, c, s):
        sw = jnp.where(even, pltpu.roll(t, DH - 1, 1), pltpu.roll(t, 1, 1))
        return (t * c + sw * s).astype(BF)

    def head(xb, h):
        qkv = jnp.dot(xb, wqkv[h], preferred_element_type=F32)
        q = rope(qkv[:, 0:DH], tab[0], tab[1])
        k = rope(qkv[:, DH:2 * DH], tab[2], tab[3])
        v = qkv[:, 2 * DH:].astype(BF)
        s = lax.dot_general(q, k, (((1,), (1,)), ((), ())), preferred_element_type=F32)
        m = jnp.max(s, axis=-1, keepdims=True)
        p = jnp.exp2(s - m)
        l = jnp.sum(p, axis=-1, keepdims=True)
        o = jnp.dot(p.astype(BF), v, preferred_element_type=F32)
        ctx[:, h * DH:(h + 1) * DH] = (o * (1.0 / l)).astype(BF)

    def attn(slot, first=False):
        xb = xg[slot]
        for h in range(HL):
            if first and h % 2 == 0:
                j = h // 2
                for t in range(3):
                    w_ld(j, t).wait()
                if j < 3:
                    for t in range(3):
                        w_ld(j + 1, t).start()
                else:
                    wo_ld.start()
                if j == 1:
                    x_ld[1].wait()
                    xg[7] = xf[1].astype(BF)
                    x_sends[0].start()
                for t in range(3):
                    for hh in range(2):
                        c0 = j * 256 + hh * DH
                        wqkv[h + hh, :, t * DH:(t + 1) * DH] = wst[t, :, c0:c0 + DH].astype(BF)
            head(xb, h)

    def p_wait(k):
        for c in range(NC):
            p_copy(k, c, right).wait_recv()

    def proj(c):
        return jnp.dot(ctx[...], wo[:, c * CW:(c + 1) * CW], preferred_element_type=F32)

    with jax.named_scope('s0'):
        attn(0, first=True)
    wo_ld.wait()
    wo[...] = wst[3].astype(BF)
    for c in range(NC):
        acc0[:, c * CW:(c + 1) * CW] = proj(c)

    def step(s, carry):
        @pl.when(s == 1)
        def _():
            x_sends[0].wait_recv()
            x_sends[2].start()
            x_sends[1].wait_recv()
            x_sends[3].start()
            x_sends[4].start()
            x_sends[5].start()

        @pl.when(s >= 3)
        def _():
            x_copy(0, s, right, 0).wait_recv()

        @pl.when(s >= 5)
        def _():
            p_wait(s - 3)

        attn(s)
        add_slot = jnp.where(s >= 5, s - 3, 6)
        for c in range(NC):
            cols = slice(c * CW, (c + 1) * CW)
            sbuf[s - 1, :, cols] = (proj(c) + rbuf[add_slot, :, cols].astype(F32)).astype(BF)
            p_copy(s - 1, c, jnp.where(s % 2 == 1, left, right)).start()
        return carry

    with jax.named_scope('loop'):
        lax.fori_loop(1, 7, step, 0)

    p_wait(1)
    p_wait(4)
    out_ref[0] = (acc0[...] + rbuf[1].astype(F32) + rbuf[4].astype(F32)).astype(out_ref.dtype)
    with jax.named_scope('s7'):
        attn(7)
    p_wait(0)
    p_wait(5)
    for c in range(NC):
        cols = slice(c * CW, (c + 1) * CW)
        out_ref[1, :, cols] = (proj(c) + rbuf[0, :, cols].astype(F32)
                               + rbuf[5, :, cols].astype(F32)).astype(out_ref.dtype)
    for cp in x_sends:
        cp.wait_send()
    for k in range(6):
        for c in range(NC):
            p_copy(k, c, right).wait_send()


def pallas_dist_rope_attn_htp_bs_b2_sq512_d1024_hq8_dh128_kernel(x, Wq, Wk, Wv, Wo):
    any_spec = pl.BlockSpec(memory_space=pltpu.HBM)
    return pl.pallas_call(
        _body,
        out_shape=jax.ShapeDtypeStruct((2, SQ, D), F32),
        in_specs=[any_spec] * 5,
        out_specs=pl.BlockSpec(memory_space=pltpu.VMEM),
        scratch_shapes=[
            pltpu.VMEM((2, SQ, D), F32),
            pltpu.VMEM((8, SQ, D), BF),
            pltpu.VMEM((4, D, D), F32),
            pltpu.VMEM((HL, D, 3 * DH), BF),
            pltpu.VMEM((D, D), BF),
            pltpu.VMEM((4, SQ, DH), F32),
            pltpu.VMEM((SQ, D), BF),
            pltpu.VMEM((6, SQ, D), BF),
            pltpu.VMEM((7, SQ, D), BF),
            pltpu.VMEM((SQ, D), F32),
            pltpu.SemaphoreType.DMA((2,)),
            pltpu.SemaphoreType.DMA((13,)),
            pltpu.SemaphoreType.DMA((6,)),
            pltpu.SemaphoreType.DMA((8,)),
            pltpu.SemaphoreType.DMA((12,)),
            pltpu.SemaphoreType.DMA((12,)),
        ],
        compiler_params=pltpu.CompilerParams(
            collective_id=0, vmem_limit_bytes=100 * 1024 * 1024),
    )(x, Wq, Wk, Wv, Wo)
```

```python
import numpy as np
import jax
import jax.numpy as jnp
from jax import lax
from jax.experimental import pallas as pl
from jax.experimental.pallas import tpu as pltpu

N_DEV = 4
SQ = 512
D = 1024
DH = 128
NT = D // DH
G = (0, 2, 4, 6, 8)
NG = len(G) - 1
HL = 8
SCALE = 0.08838834764831843
LOG2E = 1.4426950408889634
BF = jnp.bfloat16
F32 = jnp.float32
U32 = jnp.uint32
MESH = pl.DeviceIdType.MESH


def _pack(lo, hi):
    return pltpu.bitcast(pltpu.pack_elementwise([lo, hi], packed_dtype=BF), U32)


def _halves(w):
    return [pltpu.unpack_elementwise(w, index=i, packed_dtype=BF, unpacked_dtype=F32) for i in range(2)]


def _as_bf16(w):
    return pltpu.bitcast(w, BF)


def _body(x_hbm, wq_hbm, wk_hbm, wv_hbm, wo_hbm, out_ref,
          xf, xg, wst, wqkv, wo, tab, ctx, sbuf, rbuf, acc0,
          ld_sem, w_sem, xs_sem, xr_sem, ps_sem, pr_sem):
    me = lax.axis_index("i")
    left = (me + N_DEV - 1) % N_DEV
    right = (me + 1) % N_DEV

    def load_tiles(ref, lo, hi):
        return jnp.concatenate([_as_bf16(ref[n]) for n in range(lo, hi)], axis=1)

    def store_x(slot, b):
        for n in range(NT):
            for r in range(4):
                xg[slot, n, r * SQ // 8:(r + 1) * SQ // 8, :] = _pack(
                    *(xf[b, n, pl.ds(r // 2 * (SQ // 2) + r % 2 + 2 * i, SQ // 8, stride=4), :] for i in range(2)))

    def tile_copies(src, dst, lo, hi, sem):
        return [pltpu.make_async_copy(src.at[:, pl.ds(n * DH, DH)], dst.at[n], sem) for n in range(lo, hi)]

    x_ld = [tile_copies(x_hbm.at[b], xf.at[b], 0, NT, ld_sem.at[b]) for b in range(2)]
    w_ld = [[cp for t, w in enumerate((wq_hbm, wk_hbm, wv_hbm))
             for cp in tile_copies(w, wst.at[t], G[j], G[j + 1], w_sem.at[j])] for j in range(NG)]
    wo_ld = tile_copies(wo_hbm, wst.at[3], 0, NT, w_sem.at[NG])

    for cp in x_ld[0] + w_ld[0]:
        cp.start()

    barrier = pltpu.get_barrier_semaphore()
    for nbr in (left, right):
        pl.semaphore_signal(barrier, inc=1, device_id=(nbr,), device_id_type=MESH)

    def x_copy(src_slot, dst_slot, dev, k):
        return pltpu.make_async_remote_copy(
            src_ref=xg.at[src_slot], dst_ref=xg.at[dst_slot],
            send_sem=xs_sem.at[k], recv_sem=xr_sem.at[dst_slot],
            device_id=(dev,), device_id_type=MESH)

    x_sends = [
        x_copy(7, 1, right, 0), x_copy(0, 2, left, 1),
        x_copy(1, 4, right, 2), x_copy(2, 3, left, 3),
        x_copy(0, 5, right, 4), x_copy(7, 6, left, 5),
    ]

    NC = 2
    CW = D // NC
    CT = CW // DH

    def p_copy(k, c, dev):
        cols = pl.ds(c * CT, CT)
        return pltpu.make_async_remote_copy(
            src_ref=sbuf.at[k, cols], dst_ref=rbuf.at[k, cols],
            send_sem=ps_sem.at[k * NC + c], recv_sem=pr_sem.at[k * NC + c],
            device_id=(dev,), device_id_type=MESH)

    def angles(n, position):
        lane = lax.broadcasted_iota(jnp.int32, (n, DH), 1)
        row = lax.broadcasted_iota(jnp.int32, (n, DH), 0)
        inv = jnp.exp((lane // 2).astype(F32) * (-2.0 * np.log(10000.0) / DH))
        ang = position(row).astype(F32) * inv
        return jnp.cos(ang), jnp.sin(ang)

    ca, sa = (t[:, None, :] for t in angles(SQ // 8, lambda a: 256 * (a // 32) + 16 * (a % 16) + (a // 16) % 2))
    cb, sb = (t[None, :, :] for t in angles(8, lambda b: 2 * b))
    cos = (ca * cb - sa * sb).reshape(SQ, DH)
    sin = (sa * cb + ca * sb).reshape(SQ, DH)
    even = (lax.broadcasted_iota(jnp.int32, (SQ, DH), 1) % 2) == 0
    sin = jnp.where(even, -sin, sin)
    tab[0] = cos * (SCALE * LOG2E)
    tab[1] = sin * (SCALE * LOG2E)
    tab[2] = cos
    tab[3] = sin

    rbuf[6] = jnp.zeros((NT, SQ // 2, DH), U32)
    for cp in x_ld[0]:
        cp.wait()
    for cp in w_ld[1]:
        cp.start()
    store_x(0, 0)
    pl.semaphore_wait(barrier, 2)
    x_sends[1].start()
    x_sends[4].start()

    def rope(t, c, s):
        sw = jnp.where(even, pltpu.roll(t, DH - 1, 1), pltpu.roll(t, 1, 1))
        return (t * c + sw * s).astype(BF)

    HM, HK = SQ // 2, D // 2

    def x_operands(slot):
        def blk(r, c):
            return jnp.concatenate(
                [xg[slot, n, r * HM // 2:(r + 1) * HM // 2, :] for n in range(c * NT // 2, (c + 1) * NT // 2)],
                axis=1)
        w11, w12, w21, w22 = blk(0, 0), blk(0, 1), blk(1, 0), blk(1, 1)
        sums = [_pack(*pair) for pair in zip(*(
            (a11 + a22, a21 + a22, a11 + a12, a21 - a11, a12 - a22)
            for a11, a12, a21, a22 in zip(*(_halves(w) for w in (w11, w12, w21, w22)))))]
        return [_as_bf16(w) for w in (sums[0], sums[1], w11, w22, sums[2], sums[3], sums[4])]

    def prep_weights(p, t):
        c1, c2 = 2 * p, 2 * p + 1
        ops = []
        for par in range(2):
            r1, r2 = pl.ds(par, HK // 2, stride=2), pl.ds(HK + par, HK // 2, stride=2)
            b11, b12, b21, b22 = wst[t, c1, r1, :], wst[t, c2, r1, :], wst[t, c1, r2, :], wst[t, c2, r2, :]
            ops.append((b11 + b22, b11, b12 - b22, b21 - b11, b22, b11 + b12, b21 + b22))
        for i, pair in enumerate(zip(*ops)):
            wqkv[p, t, i] = _pack(*pair)

    def qkv_proj(xs, p):
        lo, hi = [], []
        for t in range(3):
            m1, m2, m3, m4, m5, m6, m7 = (
                jnp.dot(xs[i], _as_bf16(wqkv[p, t, i]), preferred_element_type=F32) for i in range(7))
            lo.append(jnp.concatenate([m1 + m4 - m5 + m7, m2 + m4], axis=0))
            hi.append(jnp.concatenate([m3 + m5, m1 - m2 + m3 + m6], axis=0))
        return [(rope(q, tab[0], tab[1]), rope(k, tab[2], tab[3]), v.astype(BF)) for q, k, v in (lo, hi)]

    def recip(l):
        r = pl.reciprocal(l, approx=True)
        return r * (2.0 - l * r)

    def head_attn(q, k, v):
        s = lax.dot_general(q, k, (((1,), (1,)), ((), ())), preferred_element_type=F32)
        m = jnp.max(s, axis=-1, keepdims=True)
        p = jnp.exp2(s - m)
        l = jnp.sum(p, axis=-1, keepdims=True)
        o = jnp.dot(p.astype(BF), v, preferred_element_type=F32)
        return o * recip(l)

    def pair_attn(p, heads):
        e, o = (head_attn(*hd) for hd in heads)
        a11, a21, a12, a22 = e[:HM], e[HM:], o[:HM], o[HM:]
        for i, a in enumerate((a11 + a22, a21 + a22, a11, a22, a11 + a12, a21 - a11, a12 - a22)):
            ctx[i, p] = _pack(a[:HM // 2], a[HM // 2:])

    def prep_wo():
        for p in range(HL // 2):
            for n in range(NT // 2):
                ops = []
                for par in range(2):
                    r1, r2 = (pl.ds((2 * p + u) * DH + par, DH // 2, stride=2) for u in range(2))
                    b11, b12 = wst[3, n, r1, :], wst[3, NT // 2 + n, r1, :]
                    b21, b22 = wst[3, n, r2, :], wst[3, NT // 2 + n, r2, :]
                    ops.append((b11 + b22, b11, b12 - b22, b21 - b11, b22, b11 + b12, b21 + b22))
                for i, pair in enumerate(zip(*ops)):
                    wo[i, n, p * DH // 2:(p + 1) * DH // 2, :] = _pack(*pair)

    def col_tiles(c):
        return (2 * c, 2 * c + 1, NT // 2 + 2 * c, NT // 2 + 2 * c + 1)

    def store_out(b, c, res):
        for u, n in enumerate(col_tiles(c)):
            out_ref[b, :, n * DH:(n + 1) * DH] = res[:, u * DH:(u + 1) * DH].astype(out_ref.dtype)

    def out_proj(c):
        a = [load_tiles(ctx.at[i], 0, HL // 2) for i in range(7)]
        lo, hi = [], []
        for n in (2 * c, 2 * c + 1):
            m1, m2, m3, m4, m5, m6, m7 = (
                jnp.dot(a[i], _as_bf16(wo[i, n]), preferred_element_type=F32) for i in range(7))
            lo.append(jnp.concatenate([m1 + m4 - m5 + m7, m2 + m4], axis=0))
            hi.append(jnp.concatenate([m3 + m5, m1 - m2 + m3 + m6], axis=0))
        return jnp.concatenate(lo + hi, axis=1)

    def attn(slot, first=False):
        xs = x_operands(slot)
        pending = None
        for h in range(0, HL, 2):
            if first and h in G:
                j = G.index(h)
                for cp in w_ld[j]:
                    cp.wait()
                if j + 2 < NG:
                    for cp in w_ld[j + 2]:
                        cp.start()
                if j == NG - 2:
                    for cp in wo_ld:
                        cp.start()
                for t in range(3):
                    prep_weights(j, t)
            cur = qkv_proj(xs, h // 2)
            if pending is not None:
                pair_attn(h // 2 - 1, pending)
            pending = cur
        if first:
            for cp in wo_ld:
                cp.wait()
            for cp in x_ld[1]:
                cp.start()
            prep_wo()
        pair_attn(HL // 2 - 1, pending)

    def p_wait(k):
        for c in range(NC):
            p_copy(k, c, right).wait_recv()

    def recvd(k, c):
        w = jnp.concatenate([rbuf[k, n] for n in range(c * CT, (c + 1) * CT)], axis=1)
        return jnp.concatenate(_halves(w), axis=0)

    attn(0, first=True)
    for c in range(NC):
        acc0[:, c * CW:(c + 1) * CW] = out_proj(c)

    def step(i, carry):
        s = jnp.where(i <= 2, i + 1, jnp.where(i == 3, 1, i))

        @pl.when(s == 1)
        def _():
            x_sends[0].wait_recv()
            x_sends[2].start()

        @pl.when(s == 2)
        def _():
            x_sends[1].wait_recv()
            x_sends[3].start()
            for cp in x_ld[1]:
                cp.wait()
            store_x(7, 1)
            x_sends[0].start()
            x_sends[5].start()

        @pl.when(s >= 3)
        def _():
            x_copy(0, s, right, 0).wait_recv()

        @pl.when(s >= 5)
        def _():
            p_wait(s - 3)

        attn(s)
        add_slot = jnp.where(s >= 5, s - 3, 6)
        for c in range(NC):
            res = out_proj(c) + recvd(add_slot, c)
            for n in range(CT):
                sbuf[s - 1, c * CT + n] = _pack(res[:HM, n * DH:(n + 1) * DH], res[HM:, n * DH:(n + 1) * DH])
            p_copy(s - 1, c, jnp.where(s % 2 == 1, left, right)).start()
        return carry

    lax.fori_loop(1, 7, step, 0)

    p_wait(1)
    p_wait(4)
    for c in range(NC):
        store_out(0, c, acc0[:, c * CW:(c + 1) * CW] + recvd(1, c) + recvd(4, c))
    attn(7)
    for c in range(NC):
        res = out_proj(c)
        p_copy(0, c, right).wait_recv()
        p_copy(5, c, right).wait_recv()
        store_out(1, c, res + recvd(0, c) + recvd(5, c))
    for cp in x_sends:
        cp.wait_send()
    for k in range(6):
        for c in range(NC):
            p_copy(k, c, right).wait_send()


def pallas_dist_rope_attn_htp_bs_b2_sq512_d1024_hq8_dh128_kernel(x, Wq, Wk, Wv, Wo):
    any_spec = pl.BlockSpec(memory_space=pltpu.HBM)
    return pl.pallas_call(
        _body,
        out_shape=jax.ShapeDtypeStruct((2, SQ, D), BF),
        in_specs=[any_spec] * 5,
        out_specs=pl.BlockSpec(memory_space=pltpu.VMEM),
        scratch_shapes=[
            pltpu.VMEM((2, NT, SQ, DH), F32),
            pltpu.VMEM((8, NT, SQ // 2, DH), U32),
            pltpu.VMEM((4, NT, D, DH), F32),
            pltpu.VMEM((HL // 2, 3, 7, D // 4, DH), U32),
            pltpu.VMEM((7, NT // 2, D // 4, DH), U32),
            pltpu.VMEM((4, SQ, DH), F32),
            pltpu.VMEM((7, HL // 2, SQ // 4, DH), U32),
            pltpu.VMEM((6, NT, SQ // 2, DH), U32),
            pltpu.VMEM((7, NT, SQ // 2, DH), U32),
            pltpu.VMEM((SQ, D), F32),
            pltpu.SemaphoreType.DMA((2,)),
            pltpu.SemaphoreType.DMA((NG + 1,)),
            pltpu.SemaphoreType.DMA((6,)),
            pltpu.SemaphoreType.DMA((8,)),
            pltpu.SemaphoreType.DMA((12,)),
            pltpu.SemaphoreType.DMA((12,)),
        ],
        compiler_params=pltpu.CompilerParams(
            collective_id=0, vmem_limit_bytes=100 * 1024 * 1024),
    )(x, Wq, Wk, Wv, Wo)
```
